```python
import numpy as np

kernel_name = "dist_rope_attn_qseq_b2_sq128_d512_hq4_dh64"

def setup_inputs():
    x = np.random.randn(2, 512, 512).astype(np.float32)
    Wq = np.random.randn(512, 256).astype(np.float32) * 0.02
    Wk = np.random.randn(512, 256).astype(np.float32) * 0.02
    Wv = np.random.randn(512, 256).astype(np.float32) * 0.02
    Wo = np.random.randn(256, 512).astype(np.float32) * 0.02
    return {"x": x, "Wq": Wq, "Wk": Wk, "Wv": Wv, "Wo": Wo}

def reference(x, Wq, Wk, Wv, Wo):
    B, Sq, Hq, Dh = 2, 512, 4, 64
    inv = 1.0 / (10000.0 ** (np.arange(0, Dh, 2) / Dh))
    pos = np.arange(Sq)[:, None] * inv[None, :]
    cos = np.repeat(np.cos(pos), 2, axis=-1).astype(np.float32)
    sin = np.repeat(np.sin(pos), 2, axis=-1).astype(np.float32)
    def rot(t):
        t2 = t.reshape(B, Sq, Hq, Dh // 2, 2)
        t_r = np.stack([-t2[..., 1], t2[..., 0]], axis=-1).reshape(B, Sq, Hq, Dh)
        return t * cos[None, :, None, :] + t_r * sin[None, :, None, :]
    Q = rot((x @ Wq).reshape(B, Sq, Hq, Dh))
    K = rot((x @ Wk).reshape(B, Sq, Hq, Dh))
    V = (x @ Wv).reshape(B, Sq, Hq, Dh)
    s = np.einsum('bihd,bjhd->bhij', Q, K).astype(np.float32) * 0.125
    s_max = s.max(axis=-1, keepdims=True)
    w = np.exp(s - s_max)
    w = w / w.sum(axis=-1, keepdims=True)
    ctx = np.einsum('bhij,bjhd->bihd', w, V).reshape(B, Sq, Hq * Dh)
    return ctx @ Wo
```

```python
import functools
import numpy as np
import jax
import jax.numpy as jnp
from jax import lax
from jax.experimental import pallas as pl
from jax.experimental.pallas import tpu as pltpu

N_DEV = 4
B, SL, D, HD = 2, 128, 512, 256
DH = 64
LOG2E = 1.4426950408889634
F32, BF16 = jnp.float32, jnp.bfloat16
NT = (((1,), (1,)), ((), ()))


def _rope_tables(pos0):
    lane = lax.broadcasted_iota(jnp.int32, (SL, 128), 1)
    row = lax.broadcasted_iota(jnp.int32, (SL, 128), 0)
    fi = (lane % DH) // 2
    inv = jnp.exp2(fi.astype(F32) * (-2.0 * np.log2(10000.0) / DH))
    ang = (row + pos0).astype(F32) * inv
    c, s = jnp.cos(ang), jnp.sin(ang)
    s = jnp.where(lane % 2 == 0, -s, s)
    return c, s


def _rope(t, c, s):
    lane = lax.broadcasted_iota(jnp.int32, t.shape, 1)
    sw = jnp.where(lane % 2 == 0, pltpu.roll(t, 127, 1), pltpu.roll(t, 1, 1))
    return t * c + sw * s


def kernel_body(x_hbm, wq_hbm, wk_hbm, wv_hbm, wo_hbm, o_ref,
                xf, wq, wk, wv, wo, xg, lsem, ssem, rsem):
    me = lax.axis_index("i")
    bar = pltpu.get_barrier_semaphore()
    for d in (1, 3, 2):
        pl.semaphore_signal(bar, 1, device_id=((me + d) % N_DEV,), device_id_type=pl.DeviceIdType.MESH)
    cx = pltpu.make_async_copy(x_hbm, xf, lsem.at[0]); cx.start()
    ck = pltpu.make_async_copy(wk_hbm, wk, lsem.at[1]); ck.start()
    cv = pltpu.make_async_copy(wv_hbm, wv, lsem.at[2]); cv.start()
    cq = pltpu.make_async_copy(wq_hbm, wq, lsem.at[3]); cq.start()
    co = pltpu.make_async_copy(wo_hbm, wo, lsem.at[4]); co.start()

    cx.wait()
    xb = xf[...].reshape(B * SL, D).astype(BF16)
    xg[me] = xb
    pl.semaphore_wait(bar, 3)
    sends = []
    for n, d in enumerate((1, 3, 2)):
        cp = pltpu.make_async_remote_copy(xg.at[me], xg.at[me], ssem.at[n], rsem.at[n],
                                          device_id=((me + d) % N_DEV,), device_id_type=pl.DeviceIdType.MESH)
        cp.start()
        sends.append(cp)

    lane = lax.broadcasted_iota(jnp.int32, (SL, 128), 1)
    lo = lane < DH
    c_me, s_me = _rope_tables(me * SL)
    cq.wait()
    wqb = wq[...].astype(BF16)
    q = jnp.dot(xb, wqb, preferred_element_type=F32)
    qs = {}
    for b in range(B):
        for p in range(2):
            t = _rope(q[b * SL:(b + 1) * SL, p * 128:(p + 1) * 128], c_me, s_me) * (0.125 * LOG2E)
            q0 = jnp.where(lo, t, 0.0).astype(BF16)
            q1 = jnp.where(lo, 0.0, t).astype(BF16)
            qs[b, p] = jnp.concatenate([q0, q1], axis=0)
    ck.wait(); cv.wait()
    wkb = wk[...].astype(BF16)
    wvb = wv[...].astype(BF16)

    m = {}; acc = {}; l = {}

    def colblock(xblk, c, s, first):
        k = jnp.dot(xblk, wkb, preferred_element_type=F32)
        v = jnp.dot(xblk, wvb, preferred_element_type=F32).astype(BF16)
        for b in range(B):
            for p in range(2):
                kk = _rope(k[b * SL:(b + 1) * SL, p * 128:(p + 1) * 128], c, s).astype(BF16)
                vv = v[b * SL:(b + 1) * SL, p * 128:(p + 1) * 128]
                sc = lax.dot_general(qs[b, p], kk, NT, preferred_element_type=F32)
                mb = jnp.max(sc, axis=1, keepdims=True)
                if first:
                    mn = mb
                else:
                    mn = jnp.maximum(m[b, p], mb)
                pr = jnp.exp2(sc - mn)
                ls = jnp.sum(pr, axis=1, keepdims=True)
                pv = jnp.dot(pr.astype(BF16), vv, preferred_element_type=F32)
                if first:
                    l[b, p] = ls; acc[b, p] = pv
                else:
                    a = jnp.exp2(m[b, p] - mn)
                    l[b, p] = l[b, p] * a + ls
                    acc[b, p] = acc[b, p] * a + pv
                m[b, p] = mn

    colblock(xb, c_me, s_me, True)
    for n, d in ((1, 3), (0, 1), (2, 2)):
        src = (me + N_DEV - d) % N_DEV
        sends[n].wait_recv()
        c, s = _rope_tables(src * SL)
        colblock(xg[src], c, s, False)
    co.wait()
    wob = wo[...].astype(BF16)
    for b in range(B):
        parts = []
        for p in range(2):
            o = acc[b, p] / l[b, p]
            parts.append(jnp.where(lo, o[:SL], o[SL:]))
        ctx = jnp.concatenate(parts, axis=1).astype(BF16)
        o_ref[b] = jnp.dot(ctx, wob, preferred_element_type=F32)
    for cp in sends:
        cp.wait_send()


def pallas_dist_rope_attn_qseq_b2_sq128_d512_hq4_dh64_kernel(x, Wq, Wk, Wv, Wo):
    return pl.pallas_call(
        kernel_body,
        out_shape=jax.ShapeDtypeStruct((B, SL, D), F32),
        in_specs=[pl.BlockSpec(memory_space=pl.ANY)] * 5,
        out_specs=pl.BlockSpec(memory_space=pltpu.VMEM),
        scratch_shapes=[
            pltpu.VMEM((B, SL, D), F32),
            pltpu.VMEM((D, HD), F32), pltpu.VMEM((D, HD), F32), pltpu.VMEM((D, HD), F32),
            pltpu.VMEM((HD, D), F32),
            pltpu.VMEM((N_DEV, B * SL, D), BF16),
            pltpu.SemaphoreType.DMA((5,)), pltpu.SemaphoreType.DMA((3,)), pltpu.SemaphoreType.DMA((3,)),
        ],
        compiler_params=pltpu.CompilerParams(collective_id=0),
    )(x, Wq, Wk, Wv, Wo)
```

```python
import os
import numpy as np
import jax
import jax.numpy as jnp
from jax import lax
from jax.experimental import pallas as pl
from jax.experimental.pallas import tpu as pltpu

N_DEV = 4
B, SL, D, HD = 2, 128, 512, 256
DH = 64
LOG2E = 1.4426950408889634
QSCALE = 0.125 * LOG2E
F32, BF16, U32 = jnp.float32, jnp.bfloat16, jnp.uint32
NT = (((1,), (1,)), ((), ()))
TN = (((0,), (0,)), ((), ()))
MESH = pl.DeviceIdType.MESH
SCOPES = bool(int(os.environ.get("SCOPES", "0")))
TREE = bool(int(os.environ.get("TREE", "1")))
XCH = [int(v) for v in os.environ.get("XCH", "0,32,128").split(",")]


class _Null:
    def __enter__(self): return self
    def __exit__(self, *a): return False


def scope(name):
    return jax.named_scope(name) if SCOPES else _Null()


def pk(v):
    return pltpu.bitcast(v, U32)


def upk(w):
    return pltpu.bitcast(w, BF16)


def build_tables(tab, blocks):
    lane = lax.broadcasted_iota(jnp.int32, (8, 128), 1)
    fi = (lane % DH) // 2
    inv = jnp.exp2(fi.astype(F32) * np.float32(-2.0 * np.log2(10000.0) / DH))
    th = jnp.where(lane % 2 == 0, -inv, inv)
    a_s = lax.broadcasted_iota(jnp.int32, (8, 128), 0).astype(F32) * th
    c_s, s_s = jnp.cos(a_s), jnp.sin(a_s)
    th2 = jnp.concatenate([th, th], axis=0)
    u16 = lax.broadcasted_iota(jnp.int32, (16, 128), 0) * 8
    for j, blk in enumerate(blocks):
        a_u = (u16 + blk * SL).astype(F32) * th2
        c_u, s_u = jnp.cos(a_u), jnp.sin(a_u)
        for u in range(16):
            cu, su = c_u[u:u + 1, :], s_u[u:u + 1, :]
            tab[j, 0, 8 * u:8 * u + 8, :] = cu * c_s - su * s_s
            tab[j, 1, 8 * u:8 * u + 8, :] = su * c_s + cu * s_s


def rope(t, c, s):
    lane = lax.broadcasted_iota(jnp.int32, t.shape, 1)
    sw = jnp.where(lane % 2 == 0, pltpu.roll(t, 127, 1), pltpu.roll(t, 1, 1))
    return t * c + sw * s


def kernel_body(x_hbm, wq_hbm, wk_hbm, wv_hbm, wo_hbm, o_ref,
                xf, wqf, wkf, wvf, wof,
                xb, wqb, wkb, wvt, wob, tab,
                kv, qm, xin, kvin, fkv, fqm, acc, ml, pout, pin,
                lsem, xssem, xrsem, ssem, rsem, rdy):
    me = lax.axis_index("i")
    fb = me >> 1
    sb = 1 - fb
    odd = me & 1
    nE = 1 - odd
    nL = 3 - odd
    nbr = (nE, nL)
    lane = lax.broadcasted_iota(jnp.int32, (SL, 128), 1)
    lo = lane < DH
    nxc = len(XCH) - 1

    bar = pltpu.get_barrier_semaphore()
    if TREE:
        @pl.when(me != 2)
        def _():
            for n in nbr:
                pl.semaphore_signal(bar, 1, device_id=(n,), device_id_type=MESH)
    else:
        for n in nbr:
            pl.semaphore_signal(bar, 1, device_id=(n,), device_id_type=MESH)

    if TREE:
        @pl.when(me == 2)
        def _():
            pl.semaphore_wait(bar, 2)
            for n in nbr:
                pl.semaphore_signal(rdy, 1, device_id=(n,), device_id_type=MESH)

    xc = {}
    for r in range(nxc):
        for b in range(2):
            rows = pl.ds(XCH[r], XCH[r + 1] - XCH[r])
            cp = pltpu.make_async_copy(x_hbm.at[b, rows], xf.at[b, rows], lsem.at[len(xc)])
            cp.start()
            xc[b, r] = cp
    n0 = len(xc)
    ck = pltpu.make_async_copy(wk_hbm, wkf, lsem.at[n0]); ck.start()
    cv = pltpu.make_async_copy(wv_hbm, wvf, lsem.at[n0 + 1]); cv.start()
    cq = pltpu.make_async_copy(wq_hbm, wqf, lsem.at[n0 + 2]); cq.start()
    co = pltpu.make_async_copy(wo_hbm, wof, lsem.at[n0 + 3]); co.start()

    def rcopy(src, dst_of, k, d):
        return pltpu.make_async_remote_copy(src, dst_of(fb), ssem.at[k, d], rsem.at[k, fb],
                                            device_id=(nbr[d],), device_id_type=MESH)

    def rrecv(dst, k, s):
        return pltpu.make_async_remote_copy(dst, dst, ssem.at[k, s], rsem.at[k, s],
                                            device_id=(nbr[s],), device_id_type=MESH)

    def xrows(r):
        return pl.ds(XCH[r] // 2, (XCH[r + 1] - XCH[r]) // 2)

    sx = {(d, r): pltpu.make_async_remote_copy(xb.at[d, xrows(r)], xin.at[fb, xrows(r)], xssem.at[d, r], xrsem.at[fb, r],
                                               device_id=(nbr[d],), device_id_type=MESH)
          for d in range(2) for r in range(nxc)}
    rx = {(s, r): pltpu.make_async_remote_copy(xin.at[s, xrows(r)], xin.at[s, xrows(r)], xssem.at[s, r], xrsem.at[s, r],
                                               device_id=(nbr[s],), device_id_type=MESH)
          for s in range(2) for r in range(nxc)}
    skv = [rcopy(kv.at[1 - d], lambda s: kvin.at[s], 0, d) for d in range(2)]
    rkv = [rrecv(kvin.at[s], 0, s) for s in range(2)]
    PCH = ((0, 72), (72, 64))
    spt = [[rcopy(pout.at[d, pl.ds(*PCH[c])], lambda s, c=c: pin.at[s, pl.ds(*PCH[c])], 1 + c, d) for c in range(2)]
           for d in range(2)]
    rpt = [[rrecv(pin.at[s, pl.ds(*PCH[c])], 1 + c, s) for c in range(2)] for s in range(2)]

    with scope("tables"):
        build_tables(tab, (me, nE, nL))

    def xcast(b, r):
        xc[b, r].wait()
        xb[b, xrows(r), :] = pk(xf[b, XCH[r]:XCH[r + 1], :].astype(BF16))

    with scope("xc00"):
        xcast(0, 0)
    with scope("barrier"):
        if TREE:
            @pl.when(me == 0)
            def _():
                pl.semaphore_wait(bar, 2)

            @pl.when(odd == 1)
            def _():
                pl.semaphore_wait(bar, 1)
        else:
            pl.semaphore_wait(bar, 2)
    sx[0, 0].start()
    with scope("xc10"):
        xcast(1, 0)
    if TREE:
        @pl.when(odd == 0)
        def _():
            sx[1, 0].start()
    else:
        sx[1, 0].start()
    for r in range(1, nxc):
        with scope(f"xc0{r}"):
            xcast(0, r)
        sx[0, r].start()
        with scope(f"xc1{r}"):
            xcast(1, r)
        if TREE:
            @pl.when(odd == 0)
            def _():
                sx[1, r].start()
        else:
            sx[1, r].start()
    if TREE:
        @pl.when(odd == 1)
        def _():
            with scope("rdy"):
                pl.semaphore_wait(rdy, 1)
            for r in range(nxc):
                sx[1, r].start()

    def proj_k(xv, dst, tj):
        for p in range(2):
            t = jnp.dot(xv, upk(wkb[:, p * 128:(p + 1) * 128]), preferred_element_type=F32)
            dst[0, :, p * 128:(p + 1) * 128] = pk(rope(t, tab[tj, 0], tab[tj, 1]).astype(BF16))

    def proj_vt(xv, dst):
        for p in range(2):
            t = lax.dot_general(upk(wvt[p * 64:(p + 1) * 64, :]), xv, NT, preferred_element_type=F32)
            dst[1, :, p * 128:(p + 1) * 128] = pk(t.astype(BF16))

    def proj_q(xv, dst, tj):
        for p in range(2):
            t = jnp.dot(xv, upk(wqb[:, p * 128:(p + 1) * 128]), preferred_element_type=F32)
            t = rope(t, tab[tj, 0], tab[tj, 1])
            dst[p, 0] = pk(jnp.where(lo, t, 0.0).astype(BF16))
            dst[p, 1] = pk(jnp.where(lo, 0.0, t).astype(BF16))

    with scope("wait_wk"):
        ck.wait()
    wkb[...] = pk(wkf[...].astype(BF16))
    with scope("own_k"):
        for b in (1, 0):
            proj_k(upk(xb[b]), kv.at[b], 0)
    with scope("wait_wv"):
        cv.wait()
    with scope("own_v"):
        wvt[...] = pk(wvf[...].T.astype(BF16))
        for b in (1, 0):
            proj_vt(upk(xb[b]), kv.at[b])
    for d in range(2):
        skv[d].start()

    with scope("wait_wq"):
        cq.wait()
    with scope("own_q"):
        wqb[...] = pk((wqf[...] * np.float32(QSCALE)).astype(BF16))
        for b in range(2):
            proj_q(upk(xb[b]), qm.at[b], 0)

    def scores(ksrcs, qmask, p):
        k = jnp.concatenate([s[0, :, p * 128:(p + 1) * 128] for s in ksrcs], axis=0)
        return lax.dot_general(upk(k), upk(qmask), NT, preferred_element_type=F32)

    def pv(ksrcs, pt, p, hh):
        v = jnp.concatenate([upk(s[1, hh * 32:(hh + 1) * 32, p * 128:(p + 1) * 128]) for s in ksrcs], axis=1)
        return jnp.dot(v, pt, preferred_element_type=F32)

    HEADS = [(p, hh) for p in range(2) for hh in range(2)]

    def own_update(bs, ksrcs_of, first):
        grp = [(b, p, hh) for b in bs for (p, hh) in HEADS]
        ss = [scores(ksrcs_of(b), qm[b, p, hh], p) for (b, p, hh) in grp]
        soft = []
        for i, (b, p, hh) in enumerate(grp):
            g = 2 * p + hh
            s = ss[i]
            mb = jnp.max(s, axis=0, keepdims=True)
            if first:
                mn = mb
            else:
                mo = ml[b, g:g + 1, :]
                mn = jnp.maximum(mo, mb)
            pr = jnp.exp2(s - mn)
            ls = jnp.sum(pr, axis=0, keepdims=True)
            a = None
            if not first:
                a = jnp.exp2(mo - mn)
                ls = ml[b, 4 + g:5 + g, :] * a + ls
            ml[b, g:g + 1, :] = mn
            ml[b, 4 + g:5 + g, :] = ls
            soft.append((pr.astype(BF16), a))
        for i, (b, p, hh) in enumerate(grp):
            g = 2 * p + hh
            pr, a = soft[i]
            o = pv(ksrcs_of(b), pr, p, hh)
            if not first:
                o = acc[b, g * DH:(g + 1) * DH, :] * a + o
            acc[b, g * DH:(g + 1) * DH, :] = o

    with scope("own_attn"):
        own_update((0, 1), lambda b: [kv.at[b]], True)

    srow = lax.broadcasted_iota(jnp.int32, (8, 128), 0)

    def partial(d):
        src = [fkv.at[1 - d]]
        ss = {k_: scores(src, fqm[d, k_[0], k_[1]], k_[0]) for k_ in HEADS}
        st = jnp.zeros((8, 128), F32)
        prs = {}
        for (p, hh) in HEADS:
            g = 2 * p + hh
            s = ss[p, hh]
            mb = jnp.max(s, axis=0, keepdims=True)
            pr = jnp.exp2(s - mb)
            ls = jnp.sum(pr, axis=0, keepdims=True)
            prs[p, hh] = pr.astype(BF16)
            st = jnp.where(srow == g, mb, st)
            st = jnp.where(srow == 4 + g, ls, st)
        pout[d, 0:8, :] = pltpu.bitcast(st, U32)
        for (p, hh) in HEADS:
            g = 2 * p + hh
            pout[d, 8 + g * 32:8 + (g + 1) * 32, :] = pk(pv(src, prs[p, hh], p, hh).astype(BF16))
        for c in range(2):
            spt[d][c].start()

    with scope("wait_xE"):
        for r in range(nxc):
            rx[0, r].wait_recv()
    with scope("proj_E"):
        xe = upk(xin[0])
        proj_q(xe, fqm.at[0], 1)
        proj_k(xe, fkv.at[0], 1)
        proj_vt(xe, fkv.at[0])
    with scope("wait_xL"):
        for r in range(nxc):
            rx[1, r].wait_recv()
    with scope("part_E"):
        xl = upk(xin[1])
        proj_k(xl, fkv.at[1], 2)
        proj_vt(xl, fkv.at[1])
        partial(0)
    with scope("part_L"):
        proj_q(upk(xin[1]), fqm.at[1], 2)
        partial(1)

    with scope("attn_fb"):
        own_update((fb,), lambda b: [fkv.at[0], fkv.at[1]], False)
    with scope("wait_wo"):
        co.wait()
    wob[...] = pk(wof[...].astype(BF16))
    with scope("wait_kv"):
        for s in range(2):
            rkv[s].wait_recv()
    with scope("attn_sb"):
        own_update((sb,), lambda b: [kvin.at[0], kvin.at[1]], False)

    with scope("wait_p0"):
        for b in range(2):
            rpt[b][0].wait_recv()
    with scope("final0"):
        fac = []
        for b in range(2):
            rem = pltpu.bitcast(pin[b, 0:8, :], F32)
            own = ml[b]
            mn = jnp.maximum(own, rem)
            a_o = jnp.exp2(own - mn)
            a_r = jnp.exp2(rem - mn)
            l = a_o * pltpu.roll(own, 4, 0) + a_r * pltpu.roll(rem, 4, 0)
            inv = 1.0 / l
            fac.append((a_o * inv, a_r * inv))

    def ctx_pair(p):
        cols = []
        for b in range(2):
            f_o, f_r = fac[b]
            parts = []
            for g in (2 * p, 2 * p + 1):
                parts.append(acc[b, g * DH:(g + 1) * DH, :] * f_o[g:g + 1, :]
                             + upk(pin[b, 8 + g * 32:8 + (g + 1) * 32, :]).astype(F32) * f_r[g:g + 1, :])
            cols.append(jnp.concatenate(parts, axis=0).astype(BF16))
        return jnp.concatenate(cols, axis=1)

    with scope("final0b"):
        o0 = lax.dot_general(ctx_pair(0), upk(wob[0:64, :]), TN, preferred_element_type=F32)
        o_ref[...] = o0.reshape(B, SL, D)
    with scope("wait_p1"):
        for b in range(2):
            rpt[b][1].wait_recv()
    with scope("final1"):
        o1 = lax.dot_general(ctx_pair(1), upk(wob[64:128, :]), TN, preferred_element_type=F32)
        o_ref[...] = o_ref[...] + o1.reshape(B, SL, D)
    with scope("drain"):
        for cp in list(sx.values()) + skv + spt[0] + spt[1]:
            cp.wait_send()


def pallas_dist_rope_attn_qseq_b2_sq128_d512_hq4_dh64_kernel(x, Wq, Wk, Wv, Wo):
    nxc = len(XCH) - 1
    return pl.pallas_call(
        kernel_body,
        out_shape=jax.ShapeDtypeStruct((B, SL, D), F32),
        in_specs=[pl.BlockSpec(memory_space=pl.ANY)] * 5,
        out_specs=pl.BlockSpec(memory_space=pltpu.VMEM),
        scratch_shapes=[
            pltpu.VMEM((B, SL, D), F32),
            pltpu.VMEM((D, HD), F32), pltpu.VMEM((D, HD), F32), pltpu.VMEM((D, HD), F32), pltpu.VMEM((HD, D), F32),
            pltpu.VMEM((B, SL // 2, D), U32),
            pltpu.VMEM((D // 2, HD), U32), pltpu.VMEM((D // 2, HD), U32),
            pltpu.VMEM((HD // 2, D), U32), pltpu.VMEM((HD // 2, D), U32),
            pltpu.VMEM((3, 2, SL, 128), F32),
            pltpu.VMEM((2, 2, SL // 2, HD), U32),
            pltpu.VMEM((2, 2, 2, SL // 2, 128), U32),
            pltpu.VMEM((2, SL // 2, D), U32),
            pltpu.VMEM((2, 2, SL // 2, HD), U32),
            pltpu.VMEM((2, 2, SL // 2, HD), U32),
            pltpu.VMEM((2, 2, 2, SL // 2, 128), U32),
            pltpu.VMEM((2, HD, SL), F32),
            pltpu.VMEM((2, 8, SL), F32),
            pltpu.VMEM((2, HD // 2 + 8, SL), U32),
            pltpu.VMEM((2, HD // 2 + 8, SL), U32),
            pltpu.SemaphoreType.DMA((2 * nxc + 4,)),
            pltpu.SemaphoreType.DMA((2, nxc)), pltpu.SemaphoreType.DMA((2, nxc)),
            pltpu.SemaphoreType.DMA((3, 2)), pltpu.SemaphoreType.DMA((3, 2)),
            pltpu.SemaphoreType.REGULAR,
        ],
        compiler_params=pltpu.CompilerParams(collective_id=0),
    )(x, Wq, Wk, Wv, Wo)
```

```python
import functools

import numpy as np
import jax
import jax.numpy as jnp
from jax import lax
from jax.experimental import pallas as pl
from jax.experimental.pallas import tpu as pltpu

B, SL, D, HD = 2, 128, 512, 256
DH = 64
QSCALE = np.float32(0.125 * 1.4426950408889634)
F32, BF16, U32 = jnp.float32, jnp.bfloat16, jnp.uint32
NT = (((1,), (1,)), ((), ()))
TN = (((0,), (0,)), ((), ()))
MESH = pl.DeviceIdType.MESH
XCH = (0, 16, 48, 128)
NXC = len(XCH) - 1
HEADS = tuple((p, hh) for p in range(2) for hh in range(2))
PCH = ((0, 72), (72, 64))


def pk(v):
    return pltpu.bitcast(v, U32)


def upk(w):
    return pltpu.bitcast(w, BF16)


def cast_store(dst, src, r0, r1, scale=None):
    for c in range(src.shape[-1] // 128):
        v = src[r0:r1, c * 128:(c + 1) * 128]
        if scale is not None:
            v = v * scale
        dst[r0 // 2:r1 // 2, c * 128:(c + 1) * 128] = pk(v.astype(BF16))


def build_tables(tab, blocks):
    lane = lax.broadcasted_iota(jnp.int32, (8, 128), 1)
    fi = (lane % DH) // 2
    inv = jnp.exp2(fi.astype(F32) * np.float32(-2.0 * np.log2(10000.0) / DH))
    th = jnp.where(lane % 2 == 0, -inv, inv)
    a_s = lax.broadcasted_iota(jnp.int32, (8, 128), 0).astype(F32) * th
    c_s, s_s = jnp.cos(a_s), jnp.sin(a_s)
    th2 = jnp.concatenate([th, th], axis=0)
    u16 = lax.broadcasted_iota(jnp.int32, (16, 128), 0) * 8
    for j, blk in enumerate(blocks):
        a_u = (u16 + blk * SL).astype(F32) * th2
        c_u, s_u = jnp.cos(a_u), jnp.sin(a_u)
        for u in range(16):
            cu, su = c_u[u:u + 1, :], s_u[u:u + 1, :]
            tab[j, 0, 8 * u:8 * u + 8, :] = cu * c_s - su * s_s
            tab[j, 1, 8 * u:8 * u + 8, :] = su * c_s + cu * s_s


def rope(t, c, s):
    lane = lax.broadcasted_iota(jnp.int32, t.shape, 1)
    swapped = jnp.where(lane % 2 == 0, pltpu.roll(t, 127, 1), pltpu.roll(t, 1, 1))
    return t * c + swapped * s


def _kernel(x_hbm, wq_hbm, wk_hbm, wv_hbm, wo_hbm, o_ref,
            xf, wqf, wkf, wvf, wof,
            xb, wqb, wkb, wvt, wob, tab,
            kv, qm, xin, kvin, fkv, fqm, acc, ml, pout, pin,
            ssem, rsem, rdy):
    me = lax.axis_index("i")
    fb = me >> 1
    sb = 1 - fb
    odd = me & 1
    nbr = (1 - odd, 3 - odd)
    lo = lax.broadcasted_iota(jnp.int32, (SL, 128), 1) < DH

    def rcopy(src, dst, k, d):
        return pltpu.make_async_remote_copy(src, dst, ssem, rsem.at[k],
                                            device_id=(nbr[d],), device_id_type=MESH)

    def rwait(dst, k):
        pltpu.make_async_copy(dst, dst, rsem.at[k]).wait()

    def xrows(r):
        return pl.ds(XCH[r] // 2, (XCH[r + 1] - XCH[r]) // 2)

    sx = {(d, r): rcopy(xb.at[d, xrows(r)], xin.at[fb, xrows(r)], fb, d)
          for d in range(2) for r in range(NXC)}
    skv = [rcopy(kv.at[1 - d], kvin.at[fb], 2, d) for d in range(2)]
    spt = [[rcopy(pout.at[d, pl.ds(*PCH[c])], pin.at[fb, pl.ds(*PCH[c])], 3 + c, d) for c in range(2)]
           for d in range(2)]

    def proj_k(xv, dst, tj):
        for p in range(2):
            t = jnp.dot(xv, upk(wkb[:, p * 128:(p + 1) * 128]), preferred_element_type=F32)
            dst[0, :, p * 128:(p + 1) * 128] = pk(rope(t, tab[tj, 0], tab[tj, 1]).astype(BF16))

    def proj_vt(xv, dst):
        for p in range(2):
            t = lax.dot_general(upk(wvt[p * 64:(p + 1) * 64, :]), xv, NT, preferred_element_type=F32)
            dst[1, :, p * 128:(p + 1) * 128] = pk(t.astype(BF16))

    def proj_q(xv, dst, tj):
        for p in range(2):
            t = jnp.dot(xv, upk(wqb[:, p * 128:(p + 1) * 128]), preferred_element_type=F32)
            t = rope(t, tab[tj, 0], tab[tj, 1])
            dst[p, 0] = pk(jnp.where(lo, t, 0.0).astype(BF16))
            dst[p, 1] = pk(jnp.where(lo, 0.0, t).astype(BF16))

    def scores(ksrcs, qmask, p):
        k = jnp.concatenate([s[0, :, p * 128:(p + 1) * 128] for s in ksrcs], axis=0)
        return lax.dot_general(upk(k), upk(qmask), NT, preferred_element_type=F32)

    def pv(ksrcs, pt, p, hh):
        v = jnp.concatenate([upk(s[1, hh * 32:(hh + 1) * 32, p * 128:(p + 1) * 128]) for s in ksrcs], axis=1)
        return jnp.dot(v, pt, preferred_element_type=F32)

    def own_update(bs, ksrcs_of, first):
        grp = [(b, p, hh) for b in bs for (p, hh) in HEADS]
        ss = [scores(ksrcs_of(b), qm[b, p, hh], p) for (b, p, hh) in grp]
        soft = []
        for i, (b, p, hh) in enumerate(grp):
            g = 2 * p + hh
            s = ss[i]
            mb = jnp.max(s, axis=0, keepdims=True)
            if first:
                mn = mb
            else:
                mo = ml[b, g:g + 1, :]
                mn = jnp.maximum(mo, mb)
            pr = jnp.exp2(s - mn)
            ls = jnp.sum(pr, axis=0, keepdims=True)
            a = None
            if not first:
                a = jnp.exp2(mo - mn)
                ls = ml[b, 4 + g:5 + g, :] * a + ls
            ml[b, g:g + 1, :] = mn
            ml[b, 4 + g:5 + g, :] = ls
            soft.append((pr.astype(BF16), a))
        for i, (b, p, hh) in enumerate(grp):
            g = 2 * p + hh
            pr, a = soft[i]
            o = pv(ksrcs_of(b), pr, p, hh)
            if not first:
                o = acc[b, g * DH:(g + 1) * DH, :] * a + o
            acc[b, g * DH:(g + 1) * DH, :] = o

    @functools.partial(pl.run_scoped, lsem=pltpu.SemaphoreType.DMA((2 * NXC + 4,)))
    def _(lsem):
        bar = pltpu.get_barrier_semaphore()

        @pl.when(me != 2)
        def _():
            for n in nbr:
                pl.semaphore_signal(bar, 1, device_id=(n,), device_id_type=MESH)

        @pl.when(me == 2)
        def _():
            pl.semaphore_wait(bar, 2)
            for n in nbr:
                pl.semaphore_signal(rdy, 1, device_id=(n,), device_id_type=MESH)

        xc = {}
        for r in range(NXC):
            for b in range(2):
                rows = pl.ds(XCH[r], XCH[r + 1] - XCH[r])
                cp = pltpu.make_async_copy(x_hbm.at[b, rows], xf.at[b, rows], lsem.at[len(xc)])
                cp.start()
                xc[b, r] = cp
        n0 = len(xc)
        ck = pltpu.make_async_copy(wk_hbm, wkf, lsem.at[n0])
        cv = pltpu.make_async_copy(wv_hbm, wvf, lsem.at[n0 + 1])
        cq = pltpu.make_async_copy(wq_hbm, wqf, lsem.at[n0 + 2])
        co = pltpu.make_async_copy(wo_hbm, wof, lsem.at[n0 + 3])
        for cp in (ck, cv, cq, co):
            cp.start()

        build_tables(tab, (me,) + nbr)

        def xcast(b, r):
            xc[b, r].wait()
            cast_store(xb.at[b], xf.at[b], XCH[r], XCH[r + 1])

        xcast(0, 0)

        @pl.when(me == 0)
        def _():
            pl.semaphore_wait(bar, 2)

        @pl.when(odd == 1)
        def _():
            pl.semaphore_wait(bar, 1)

        for r in range(NXC):
            if r > 0:
                xcast(0, r)
            sx[0, r].start()
            xcast(1, r)

            @pl.when(odd == 0)
            def _():
                sx[1, r].start()

        @pl.when(odd == 1)
        def _():
            pl.semaphore_wait(rdy, 1)
            for r in range(NXC):
                sx[1, r].start()

        ck.wait()
        cast_store(wkb, wkf, 0, D)
        for b in (1, 0):
            proj_k(upk(xb[b]), kv.at[b], 0)
        cv.wait()
        for c in range(4):
            wvt[:, c * 128:(c + 1) * 128] = pk(wvf[c * 128:(c + 1) * 128, :].T.astype(BF16))
        proj_vt(upk(xb[1]), kv.at[1])
        skv[0].start()
        proj_vt(upk(xb[0]), kv.at[0])
        skv[1].start()

        cq.wait()
        cast_store(wqb, wqf, 0, D, QSCALE)
        for b in range(2):
            proj_q(upk(xb[b]), qm.at[b], 0)
        own_update((0, 1), lambda b: [kv.at[b]], True)
        co.wait()
        cast_store(wob, wof, 0, HD)

    srow = lax.broadcasted_iota(jnp.int32, (8, 128), 0)

    def partial(d):
        src = [fkv.at[1 - d]]
        ss = [scores(src, fqm[d, p, hh], p) for (p, hh) in HEADS]
        st = jnp.zeros((8, 128), F32)
        prs = []
        for g, s in enumerate(ss):
            mb = jnp.max(s, axis=0, keepdims=True)
            pr = jnp.exp2(s - mb)
            ls = jnp.sum(pr, axis=0, keepdims=True)
            prs.append(pr.astype(BF16))
            st = jnp.where(srow == g, mb, st)
            st = jnp.where(srow == 4 + g, ls, st)
        pout[d, 0:8, :] = pltpu.bitcast(st, U32)
        for g, (p, hh) in enumerate(HEADS):
            pout[d, 8 + g * 32:8 + (g + 1) * 32, :] = pk(pv(src, prs[g], p, hh).astype(BF16))
        for c in range(2):
            spt[d][c].start()

    rwait(xin.at[0], 0)
    xe = upk(xin[0])
    proj_q(xe, fqm.at[0], 1)
    proj_k(xe, fkv.at[0], 1)
    proj_vt(xe, fkv.at[0])
    rwait(xin.at[1], 1)
    xl = upk(xin[1])
    proj_k(xl, fkv.at[1], 2)
    proj_vt(xl, fkv.at[1])
    partial(0)
    proj_q(upk(xin[1]), fqm.at[1], 2)
    partial(1)

    own_update((fb,), lambda b: [fkv.at[0], fkv.at[1]], False)
    rwait(kvin, 2)
    own_update((sb,), lambda b: [kvin.at[0], kvin.at[1]], False)

    rwait(pin.at[:, pl.ds(*PCH[0])], 3)
    fac = []
    for b in range(2):
        rem = pltpu.bitcast(pin[b, 0:8, :], F32)
        own = ml[b]
        mn = jnp.maximum(own, rem)
        a_o = jnp.exp2(own - mn)
        a_r = jnp.exp2(rem - mn)
        inv = 1.0 / (a_o * pltpu.roll(own, 4, 0) + a_r * pltpu.roll(rem, 4, 0))
        fac.append((a_o * inv, a_r * inv))

    def ctx_pair(p):
        cols = []
        for b in range(2):
            f_o, f_r = fac[b]
            parts = []
            for g in (2 * p, 2 * p + 1):
                parts.append(acc[b, g * DH:(g + 1) * DH, :] * f_o[g:g + 1, :]
                             + upk(pin[b, 8 + g * 32:8 + (g + 1) * 32, :]).astype(F32) * f_r[g:g + 1, :])
            cols.append(jnp.concatenate(parts, axis=0).astype(BF16))
        return jnp.concatenate(cols, axis=1)

    o0 = lax.dot_general(ctx_pair(0), upk(wob[0:64, :]), TN, preferred_element_type=F32)
    o_ref[...] = o0.reshape(B, SL, D)
    rwait(pin.at[:, pl.ds(*PCH[1])], 4)
    o1 = lax.dot_general(ctx_pair(1), upk(wob[64:128, :]), TN, preferred_element_type=F32)
    o_ref[...] = o_ref[...] + o1.reshape(B, SL, D)

    for cp in list(sx.values()) + skv + spt[0] + spt[1]:
        cp.wait_send()


def pallas_dist_rope_attn_qseq_b2_sq128_d512_hq4_dh64_kernel(x, Wq, Wk, Wv, Wo):
    return pl.pallas_call(
        _kernel,
        out_shape=jax.ShapeDtypeStruct((B, SL, D), F32),
        in_specs=[pl.BlockSpec(memory_space=pl.ANY)] * 5,
        out_specs=pl.BlockSpec(memory_space=pltpu.VMEM),
        scratch_shapes=[
            pltpu.VMEM((B, SL, D), F32),
            pltpu.VMEM((D, HD), F32),
            pltpu.VMEM((D, HD), F32),
            pltpu.VMEM((D, HD), F32),
            pltpu.VMEM((HD, D), F32),
            pltpu.VMEM((B, SL // 2, D), U32),
            pltpu.VMEM((D // 2, HD), U32),
            pltpu.VMEM((D // 2, HD), U32),
            pltpu.VMEM((HD // 2, D), U32),
            pltpu.VMEM((HD // 2, D), U32),
            pltpu.VMEM((3, 2, SL, 128), F32),
            pltpu.VMEM((2, 2, SL // 2, HD), U32),
            pltpu.VMEM((2, 2, 2, SL // 2, 128), U32),
            pltpu.VMEM((2, SL // 2, D), U32),
            pltpu.VMEM((2, 2, SL // 2, HD), U32),
            pltpu.VMEM((2, 2, SL // 2, HD), U32),
            pltpu.VMEM((2, 2, 2, SL // 2, 128), U32),
            pltpu.VMEM((2, HD, SL), F32),
            pltpu.VMEM((2, 8, SL), F32),
            pltpu.VMEM((2, HD // 2 + 8, SL), U32),
            pltpu.VMEM((2, HD // 2 + 8, SL), U32),
            pltpu.SemaphoreType.DMA,
            pltpu.SemaphoreType.DMA((5,)),
            pltpu.SemaphoreType.REGULAR,
        ],
        compiler_params=pltpu.CompilerParams(collective_id=0),
    )(x, Wq, Wk, Wv, Wo)
```

```python
import functools

import numpy as np
import jax
import jax.numpy as jnp
from jax import lax
from jax.experimental import pallas as pl
from jax.experimental.pallas import tpu as pltpu

B, SL, D, HD = 2, 128, 512, 256
DH = 64
QSCALE = np.float32(0.125 * 1.4426950408889634)
F32, BF16, U32 = jnp.float32, jnp.bfloat16, jnp.uint32
NT = (((1,), (1,)), ((), ()))
TN = (((0,), (0,)), ((), ()))
MESH = pl.DeviceIdType.MESH
XCH = (0, 16, 48, 128)
NXC = len(XCH) - 1
HEADS = tuple((p, hh) for p in range(2) for hh in range(2))
PCH = ((0, 72), (72, 64))


def pk(v):
    return pltpu.bitcast(v, U32)


def upk(w):
    return pltpu.bitcast(w, BF16)


def cast_store(dst, src, r0, r1, scale=None):
    for c in range(src.shape[-1] // 128):
        v = src[r0:r1, c * 128:(c + 1) * 128]
        if scale is not None:
            v = v * scale
        dst[r0 // 2:r1 // 2, c * 128:(c + 1) * 128] = pk(v.astype(BF16))


def build_tables(tab, blocks):
    lane = lax.broadcasted_iota(jnp.int32, (8, 128), 1)
    fi = (lane % DH) // 2
    inv = jnp.exp2(fi.astype(F32) * np.float32(-2.0 * np.log2(10000.0) / DH))
    th = jnp.where(lane % 2 == 0, -inv, inv)
    a_s = lax.broadcasted_iota(jnp.int32, (8, 128), 0).astype(F32) * th
    c_s, s_s = jnp.cos(a_s), jnp.sin(a_s)
    th2 = jnp.concatenate([th, th], axis=0)
    u16 = lax.broadcasted_iota(jnp.int32, (16, 128), 0) * 8
    for j, blk in enumerate(blocks):
        a_u = (u16 + blk * SL).astype(F32) * th2
        c_u, s_u = jnp.cos(a_u), jnp.sin(a_u)
        for u in range(16):
            cu, su = c_u[u:u + 1, :], s_u[u:u + 1, :]
            tab[j, 0, 8 * u:8 * u + 8, :] = cu * c_s - su * s_s
            tab[j, 1, 8 * u:8 * u + 8, :] = su * c_s + cu * s_s


def rope(t, c, s):
    lane = lax.broadcasted_iota(jnp.int32, t.shape, 1)
    swapped = jnp.where(lane % 2 == 0, pltpu.roll(t, 127, 1), pltpu.roll(t, 1, 1))
    return t * c + swapped * s


def _kernel(x_hbm, wq_hbm, wk_hbm, wv_hbm, wo_hbm, o_ref,
            xf, wqf, wkf, wvf, wof,
            xb, wqb, wkb, wvt, wob, tab,
            kv, qm, xin, kvin, fkv, fqm, acc, ml, pout, pin,
            ssem, rsem, rdy):
    me = lax.axis_index("i")
    fb = me >> 1
    sb = 1 - fb
    odd = me & 1
    nbr = (1 - odd, 3 - odd)
    lo = lax.broadcasted_iota(jnp.int32, (SL, 128), 1) < DH

    def rcopy(src, dst, k, d):
        return pltpu.make_async_remote_copy(src, dst, ssem, rsem.at[k],
                                            device_id=(nbr[d],), device_id_type=MESH)

    def rwait(dst, k):
        pltpu.make_async_copy(dst, dst, rsem.at[k]).wait()

    def xrows(r):
        return pl.ds(XCH[r] // 2, (XCH[r + 1] - XCH[r]) // 2)

    sx = {(d, r): rcopy(xb.at[d, xrows(r)], xin.at[fb, xrows(r)], fb, d)
          for d in range(2) for r in range(NXC)}
    skv = [rcopy(kv.at[1 - d], kvin.at[fb], 2, d) for d in range(2)]
    spt = [[rcopy(pout.at[d, pl.ds(*PCH[c])], pin.at[fb, pl.ds(*PCH[c])], 3 + c, d) for c in range(2)]
           for d in range(2)]

    def proj_k(xv, dst, tj):
        for p in range(2):
            t = jnp.dot(xv, upk(wkb[:, p * 128:(p + 1) * 128]), preferred_element_type=F32)
            dst[0, :, p * 128:(p + 1) * 128] = pk(rope(t, tab[tj, 0], tab[tj, 1]).astype(BF16))

    def proj_vt(xv, dst):
        for p in range(2):
            t = lax.dot_general(upk(wvt[p * 64:(p + 1) * 64, :]), xv, NT, preferred_element_type=F32)
            dst[1, :, p * 128:(p + 1) * 128] = pk(t.astype(BF16))

    def proj_q(xv, dst, tj):
        for p in range(2):
            t = jnp.dot(xv, upk(wqb[:, p * 128:(p + 1) * 128]), preferred_element_type=F32)
            t = rope(t, tab[tj, 0], tab[tj, 1])
            dst[p, 0] = pk(jnp.where(lo, t, 0.0).astype(BF16))
            dst[p, 1] = pk(jnp.where(lo, 0.0, t).astype(BF16))

    def scores(ksrcs, qmask, p):
        k = jnp.concatenate([s[0, :, p * 128:(p + 1) * 128] for s in ksrcs], axis=0)
        return lax.dot_general(upk(k), upk(qmask), NT, preferred_element_type=F32)

    def pv(ksrcs, pt, p, hh):
        v = jnp.concatenate([upk(s[1, hh * 32:(hh + 1) * 32, p * 128:(p + 1) * 128]) for s in ksrcs], axis=1)
        return jnp.dot(v, pt, preferred_element_type=F32)

    def own_update(bs, ksrcs_of, first):
        grp = [(b, p, hh) for b in bs for (p, hh) in HEADS]
        ss = [scores(ksrcs_of(b), qm[b, p, hh], p) for (b, p, hh) in grp]
        soft = []
        for i, (b, p, hh) in enumerate(grp):
            g = 2 * p + hh
            s = ss[i]
            mb = jnp.max(s, axis=0, keepdims=True)
            if first:
                mn = mb
            else:
                mo = ml[b, g:g + 1, :]
                mn = jnp.maximum(mo, mb)
            pr = jnp.exp2(s - mn)
            ls = jnp.sum(pr, axis=0, keepdims=True)
            a = None
            if not first:
                a = jnp.exp2(mo - mn)
                ls = ml[b, 4 + g:5 + g, :] * a + ls
            ml[b, g:g + 1, :] = mn
            ml[b, 4 + g:5 + g, :] = ls
            soft.append((pr.astype(BF16), a))
        for i, (b, p, hh) in enumerate(grp):
            g = 2 * p + hh
            pr, a = soft[i]
            o = pv(ksrcs_of(b), pr, p, hh)
            if not first:
                o = acc[b, g * DH:(g + 1) * DH, :] * a + o
            acc[b, g * DH:(g + 1) * DH, :] = o

    @functools.partial(pl.run_scoped, lsem=pltpu.SemaphoreType.DMA((2 * NXC + 4,)))
    def _(lsem):
        xc = {}
        for r in range(NXC):
            for b in range(2):
                rows = pl.ds(XCH[r], XCH[r + 1] - XCH[r])
                xc[b, r] = pltpu.make_async_copy(x_hbm.at[b, rows], xf.at[b, rows], lsem.at[len(xc)])
        xc[0, 0].start()
        bar = pltpu.get_barrier_semaphore()

        @pl.when(me != 2)
        def _():
            for n in nbr:
                pl.semaphore_signal(bar, 1, device_id=(n,), device_id_type=MESH)

        @pl.when(me == 2)
        def _():
            pl.semaphore_wait(bar, 2)
            for n in nbr:
                pl.semaphore_signal(rdy, 1, device_id=(n,), device_id_type=MESH)

        for k, cp in xc.items():
            if k != (0, 0):
                cp.start()
        n0 = len(xc)
        ck = pltpu.make_async_copy(wk_hbm, wkf, lsem.at[n0])
        cv = pltpu.make_async_copy(wv_hbm, wvf, lsem.at[n0 + 1])
        cq = pltpu.make_async_copy(wq_hbm, wqf, lsem.at[n0 + 2])
        co = pltpu.make_async_copy(wo_hbm, wof, lsem.at[n0 + 3])
        for cp in (ck, cv, cq, co):
            cp.start()

        build_tables(tab, (me,) + nbr)

        def xcast(b, r):
            xc[b, r].wait()
            cast_store(xb.at[b], xf.at[b], XCH[r], XCH[r + 1])

        xcast(0, 0)

        @pl.when(me == 0)
        def _():
            pl.semaphore_wait(bar, 2)

        @pl.when(odd == 1)
        def _():
            pl.semaphore_wait(bar, 1)

        for r in range(NXC):
            if r > 0:
                xcast(0, r)
            sx[0, r].start()
            xcast(1, r)

            @pl.when(odd == 0)
            def _():
                sx[1, r].start()

        @pl.when(odd == 1)
        def _():
            pl.semaphore_wait(rdy, 1)
            for r in range(NXC):
                sx[1, r].start()

        ck.wait()
        cast_store(wkb, wkf, 0, D)
        for b in (1, 0):
            proj_k(upk(xb[b]), kv.at[b], 0)
        cv.wait()
        for c in range(4):
            wvt[:, c * 128:(c + 1) * 128] = pk(wvf[c * 128:(c + 1) * 128, :].T.astype(BF16))
        proj_vt(upk(xb[1]), kv.at[1])
        skv[0].start()
        proj_vt(upk(xb[0]), kv.at[0])
        skv[1].start()

        cq.wait()
        cast_store(wqb, wqf, 0, D, QSCALE)
        for b in range(2):
            proj_q(upk(xb[b]), qm.at[b], 0)
        own_update((0, 1), lambda b: [kv.at[b]], True)
        co.wait()
        cast_store(wob, wof, 0, HD)

    srow = lax.broadcasted_iota(jnp.int32, (8, 128), 0)

    def partial(d):
        src = [fkv.at[1 - d]]
        ss = [scores(src, fqm[d, p, hh], p) for (p, hh) in HEADS]
        st = jnp.zeros((8, 128), F32)
        prs = []
        for g, s in enumerate(ss):
            mb = jnp.max(s, axis=0, keepdims=True)
            pr = jnp.exp2(s - mb)
            ls = jnp.sum(pr, axis=0, keepdims=True)
            prs.append(pr.astype(BF16))
            st = jnp.where(srow == g, mb, st)
            st = jnp.where(srow == 4 + g, ls, st)
        pout[d, 0:8, :] = pltpu.bitcast(st, U32)
        for g, (p, hh) in enumerate(HEADS):
            pout[d, 8 + g * 32:8 + (g + 1) * 32, :] = pk(pv(src, prs[g], p, hh).astype(BF16))
        for c in range(2):
            spt[d][c].start()

    rwait(xin.at[0], 0)
    xe = upk(xin[0])
    proj_q(xe, fqm.at[0], 1)
    proj_k(xe, fkv.at[0], 1)
    proj_vt(xe, fkv.at[0])
    rwait(xin.at[1], 1)
    xl = upk(xin[1])
    proj_k(xl, fkv.at[1], 2)
    proj_vt(xl, fkv.at[1])
    partial(0)
    proj_q(upk(xin[1]), fqm.at[1], 2)
    partial(1)

    own_update((fb,), lambda b: [fkv.at[0], fkv.at[1]], False)
    rwait(kvin, 2)
    own_update((sb,), lambda b: [kvin.at[0], kvin.at[1]], False)

    rwait(pin.at[:, pl.ds(*PCH[0])], 3)
    fac = []
    for b in range(2):
        rem = pltpu.bitcast(pin[b, 0:8, :], F32)
        own = ml[b]
        mn = jnp.maximum(own, rem)
        a_o = jnp.exp2(own - mn)
        a_r = jnp.exp2(rem - mn)
        inv = 1.0 / (a_o * pltpu.roll(own, 4, 0) + a_r * pltpu.roll(rem, 4, 0))
        fac.append((a_o * inv, a_r * inv))

    def ctx_pair(p):
        cols = []
        for b in range(2):
            f_o, f_r = fac[b]
            parts = []
            for g in (2 * p, 2 * p + 1):
                parts.append(acc[b, g * DH:(g + 1) * DH, :] * f_o[g:g + 1, :]
                             + upk(pin[b, 8 + g * 32:8 + (g + 1) * 32, :]).astype(F32) * f_r[g:g + 1, :])
            cols.append(jnp.concatenate(parts, axis=0))
        return jnp.concatenate(cols, axis=1).astype(BF16)

    o0 = lax.dot_general(ctx_pair(0), upk(wob[0:64, :]), TN, preferred_element_type=F32)
    o_ref[...] = o0.reshape(B, SL, D)
    for cp in list(sx.values()) + skv + spt[0] + spt[1]:
        cp.wait_send()
    rwait(pin.at[:, pl.ds(*PCH[1])], 4)
    o1 = lax.dot_general(ctx_pair(1), upk(wob[64:128, :]), TN, preferred_element_type=F32)
    o_ref[...] = o_ref[...] + o1.reshape(B, SL, D)


def pallas_dist_rope_attn_qseq_b2_sq128_d512_hq4_dh64_kernel(x, Wq, Wk, Wv, Wo):
    return pl.pallas_call(
        _kernel,
        out_shape=jax.ShapeDtypeStruct((B, SL, D), F32),
        in_specs=[pl.BlockSpec(memory_space=pl.ANY)] * 5,
        out_specs=pl.BlockSpec(memory_space=pltpu.VMEM),
        scratch_shapes=[
            pltpu.VMEM((B, SL, D), F32),
            pltpu.VMEM((D, HD), F32),
            pltpu.VMEM((D, HD), F32),
            pltpu.VMEM((D, HD), F32),
            pltpu.VMEM((HD, D), F32),
            pltpu.VMEM((B, SL // 2, D), U32),
            pltpu.VMEM((D // 2, HD), U32),
            pltpu.VMEM((D // 2, HD), U32),
            pltpu.VMEM((HD // 2, D), U32),
            pltpu.VMEM((HD // 2, D), U32),
            pltpu.VMEM((3, 2, SL, 128), F32),
            pltpu.VMEM((2, 2, SL // 2, HD), U32),
            pltpu.VMEM((2, 2, 2, SL // 2, 128), U32),
            pltpu.VMEM((2, SL // 2, D), U32),
            pltpu.VMEM((2, 2, SL // 2, HD), U32),
            pltpu.VMEM((2, 2, SL // 2, HD), U32),
            pltpu.VMEM((2, 2, 2, SL // 2, 128), U32),
            pltpu.VMEM((2, HD, SL), F32),
            pltpu.VMEM((2, 8, SL), F32),
            pltpu.VMEM((2, HD // 2 + 8, SL), U32),
            pltpu.VMEM((2, HD // 2 + 8, SL), U32),
            pltpu.SemaphoreType.DMA,
            pltpu.SemaphoreType.DMA((5,)),
            pltpu.SemaphoreType.REGULAR,
        ],
        compiler_params=pltpu.CompilerParams(collective_id=0),
    )(x, Wq, Wk, Wv, Wo)
```

```python
import functools

import numpy as np
import jax
import jax.numpy as jnp
from jax import lax
from jax.experimental import pallas as pl
from jax.experimental.pallas import tpu as pltpu

B, SL, D, HD = 2, 128, 512, 256
DH = 64
QSCALE = np.float32(0.125 * 1.4426950408889634)
F32, BF16, U32 = jnp.float32, jnp.bfloat16, jnp.uint32
NT = (((1,), (1,)), ((), ()))
MESH = pl.DeviceIdType.MESH
XCH = (0, 16, 48, 128)
NXC = len(XCH) - 1
HEADS = tuple((p, hh) for p in range(2) for hh in range(2))
PQ = (0, 48, 96, 128)
NPC = len(PQ) - 1


def pk(v):
    return pltpu.bitcast(v, U32)


def upk(w):
    return pltpu.bitcast(w, BF16)


def cast_store(dst, src, r0, r1, scale=None):
    for c in range(src.shape[-1] // 128):
        v = src[r0:r1, c * 128:(c + 1) * 128]
        if scale is not None:
            v = v * scale
        dst[r0 // 2:r1 // 2, c * 128:(c + 1) * 128] = pk(v.astype(BF16))


def build_tables(tab, blocks):
    lane = lax.broadcasted_iota(jnp.int32, (8, 128), 1)
    fi = (lane % DH) // 2
    inv = jnp.exp2(fi.astype(F32) * np.float32(-2.0 * np.log2(10000.0) / DH))
    th = jnp.where(lane % 2 == 0, -inv, inv)
    a_s = lax.broadcasted_iota(jnp.int32, (8, 128), 0).astype(F32) * th
    c_s, s_s = jnp.cos(a_s), jnp.sin(a_s)
    th2 = jnp.concatenate([th, th], axis=0)
    u16 = lax.broadcasted_iota(jnp.int32, (16, 128), 0) * 8
    for j, blk in enumerate(blocks):
        a_u = (u16 + blk * SL).astype(F32) * th2
        c_u, s_u = jnp.cos(a_u), jnp.sin(a_u)
        for u in range(16):
            cu, su = c_u[u:u + 1, :], s_u[u:u + 1, :]
            tab[j, 0, 8 * u:8 * u + 8, :] = cu * c_s - su * s_s
            tab[j, 1, 8 * u:8 * u + 8, :] = su * c_s + cu * s_s


def rope(t, c, s):
    lane = lax.broadcasted_iota(jnp.int32, t.shape, 1)
    swapped = jnp.where(lane % 2 == 0, pltpu.roll(t, 127, 1), pltpu.roll(t, 1, 1))
    return t * c + swapped * s


def _kernel(x_hbm, wq_hbm, wk_hbm, wv_hbm, wo_hbm, o_ref,
            xf, wqf, wkf, wvf, wof,
            xb, wqb, wkb, wvt, wob, tab,
            kv, qm, xin, kvin, fkv, fqm, acc, ml, pout, pin, sout, sin_, cown, frem,
            ssem, rsem, rdy):
    me = lax.axis_index("i")
    fb = me >> 1
    sb = 1 - fb
    odd = me & 1
    nbr = (1 - odd, 3 - odd)
    lo = lax.broadcasted_iota(jnp.int32, (SL, 128), 1) < DH

    def rcopy(src, dst, k, d):
        return pltpu.make_async_remote_copy(src, dst, ssem, rsem.at[k],
                                            device_id=(nbr[d],), device_id_type=MESH)

    def rwait(dst, k):
        pltpu.make_async_copy(dst, dst, rsem.at[k]).wait()

    def xrows(r):
        return pl.ds(XCH[r] // 2, (XCH[r + 1] - XCH[r]) // 2)

    sx = {(d, r): rcopy(xb.at[d, xrows(r)], xin.at[fb, xrows(r)], fb, d)
          for d in range(2) for r in range(NXC)}
    skv = [rcopy(kv.at[1 - d], kvin.at[fb], 2, d) for d in range(2)]
    def prows(c):
        return pl.ds(PQ[c] // 2, (PQ[c + 1] - PQ[c]) // 2)

    sst = [rcopy(sout.at[d], sin_.at[fb], 3 + NPC, d) for d in range(2)]
    spt = [[rcopy(pout.at[d, prows(c)], pin.at[fb, prows(c)], 3 + c, d) for c in range(NPC)] for d in range(2)]

    def proj_k(xv, dst, tj):
        for p in range(2):
            t = jnp.dot(xv, upk(wkb[:, p * 128:(p + 1) * 128]), preferred_element_type=F32)
            dst[0, :, p * 128:(p + 1) * 128] = pk(rope(t, tab[tj, 0], tab[tj, 1]).astype(BF16))

    def proj_vt(xv, dst):
        for p in range(2):
            t = lax.dot_general(upk(wvt[p * 64:(p + 1) * 64, :]), xv, NT, preferred_element_type=F32)
            dst[1, :, p * 128:(p + 1) * 128] = pk(t.astype(BF16))

    def proj_q(xv, dst, tj):
        for p in range(2):
            t = jnp.dot(xv, upk(wqb[:, p * 128:(p + 1) * 128]), preferred_element_type=F32)
            t = rope(t, tab[tj, 0], tab[tj, 1])
            dst[p, 0] = pk(jnp.where(lo, t, 0.0).astype(BF16))
            dst[p, 1] = pk(jnp.where(lo, 0.0, t).astype(BF16))

    def scores(ksrcs, qmask, p):
        k = jnp.concatenate([s[0, :, p * 128:(p + 1) * 128] for s in ksrcs], axis=0)
        return lax.dot_general(upk(k), upk(qmask), NT, preferred_element_type=F32)

    def pv(ksrcs, pt, p, hh):
        v = jnp.concatenate([upk(s[1, hh * 32:(hh + 1) * 32, p * 128:(p + 1) * 128]) for s in ksrcs], axis=1)
        return jnp.dot(v, pt, preferred_element_type=F32)

    def own_update(bs, ksrcs_of, first):
        grp = [(b, p, hh) for b in bs for (p, hh) in HEADS]
        ss = [scores(ksrcs_of(b), qm[b, p, hh], p) for (b, p, hh) in grp]
        soft = []
        for i, (b, p, hh) in enumerate(grp):
            g = 2 * p + hh
            s = ss[i]
            mb = jnp.max(s, axis=0, keepdims=True)
            if first:
                mn = mb
            else:
                mo = ml[b, g:g + 1, :]
                mn = jnp.maximum(mo, mb)
            pr = jnp.exp2(s - mn)
            ls = jnp.sum(pr, axis=0, keepdims=True)
            a = None
            if not first:
                a = jnp.exp2(mo - mn)
                ls = ml[b, 4 + g:5 + g, :] * a + ls
            ml[b, g:g + 1, :] = mn
            ml[b, 4 + g:5 + g, :] = ls
            soft.append((pr.astype(BF16), a))
        for i, (b, p, hh) in enumerate(grp):
            g = 2 * p + hh
            pr, a = soft[i]
            o = pv(ksrcs_of(b), pr, p, hh)
            if not first:
                o = acc[b, g * DH:(g + 1) * DH, :] * a + o
            acc[b, g * DH:(g + 1) * DH, :] = o

    @functools.partial(pl.run_scoped, lsem=pltpu.SemaphoreType.DMA((2 * NXC + 4,)))
    def _(lsem):
        xc = {}
        for r in range(NXC):
            for b in range(2):
                rows = pl.ds(XCH[r], XCH[r + 1] - XCH[r])
                xc[b, r] = pltpu.make_async_copy(x_hbm.at[b, rows], xf.at[b, rows], lsem.at[len(xc)])
        xc[0, 0].start()
        bar = pltpu.get_barrier_semaphore()

        @pl.when(me != 2)
        def _():
            for n in nbr:
                pl.semaphore_signal(bar, 1, device_id=(n,), device_id_type=MESH)

        @pl.when(me == 2)
        def _():
            pl.semaphore_wait(bar, 2)
            for n in nbr:
                pl.semaphore_signal(rdy, 1, device_id=(n,), device_id_type=MESH)

        for k, cp in xc.items():
            if k != (0, 0):
                cp.start()
        n0 = len(xc)
        ck = pltpu.make_async_copy(wk_hbm, wkf, lsem.at[n0])
        cv = pltpu.make_async_copy(wv_hbm, wvf, lsem.at[n0 + 1])
        cq = pltpu.make_async_copy(wq_hbm, wqf, lsem.at[n0 + 2])
        co = pltpu.make_async_copy(wo_hbm, wof, lsem.at[n0 + 3])
        for cp in (ck, cv, cq, co):
            cp.start()

        build_tables(tab, (me,) + nbr)

        def xcast(b, r):
            xc[b, r].wait()
            cast_store(xb.at[b], xf.at[b], XCH[r], XCH[r + 1])

        xcast(0, 0)

        @pl.when(me == 0)
        def _():
            pl.semaphore_wait(bar, 2)

        @pl.when(odd == 1)
        def _():
            pl.semaphore_wait(bar, 1)

        for r in range(NXC):
            if r > 0:
                xcast(0, r)
            sx[0, r].start()
            xcast(1, r)

            @pl.when(odd == 0)
            def _():
                sx[1, r].start()

        @pl.when(odd == 1)
        def _():
            pl.semaphore_wait(rdy, 1)
            for r in range(NXC):
                sx[1, r].start()

        ck.wait()
        cast_store(wkb, wkf, 0, D)
        for b in (1, 0):
            proj_k(upk(xb[b]), kv.at[b], 0)
        cv.wait()
        for c in range(4):
            wvt[:, c * 128:(c + 1) * 128] = pk(wvf[c * 128:(c + 1) * 128, :].T.astype(BF16))
        proj_vt(upk(xb[1]), kv.at[1])
        skv[0].start()
        proj_vt(upk(xb[0]), kv.at[0])
        skv[1].start()

        cq.wait()
        cast_store(wqb, wqf, 0, D, QSCALE)
        for b in range(2):
            proj_q(upk(xb[b]), qm.at[b], 0)
        own_update((0, 1), lambda b: [kv.at[b]], True)
        co.wait()
        cast_store(wob, wof, 0, HD)

    srow = lax.broadcasted_iota(jnp.int32, (8, 128), 0)

    def partial_scores(d):
        return [scores([fkv.at[1 - d]], fqm[d, p, hh], p) for (p, hh) in HEADS]

    def partial(d, ss):
        src = [fkv.at[1 - d]]
        st = jnp.zeros((8, 128), F32)
        prs = []
        for g, s in enumerate(ss):
            mb = jnp.max(s, axis=0, keepdims=True)
            pr = jnp.exp2(s - mb)
            ls = jnp.sum(pr, axis=0, keepdims=True)
            prs.append(pr.astype(BF16))
            st = jnp.where(srow == g, mb, st)
            st = jnp.where(srow == 4 + g, ls, st)
        sout[d] = st
        for p in range(2):
            o = jnp.concatenate([pv(src, prs[2 * p + hh], p, hh) for hh in range(2)], axis=0)
            pout[d, :, p * 128:(p + 1) * 128] = pk(o.astype(BF16).T)
        sst[d].start()
        for c in range(NPC):
            spt[d][c].start()

    rwait(xin.at[0], 0)
    proj_q(upk(xin[0]), fqm.at[0], 1)
    rwait(xin.at[1], 1)
    xl = upk(xin[1])
    proj_k(xl, fkv.at[1], 2)
    proj_vt(xl, fkv.at[1])
    s0 = partial_scores(0)
    proj_q(upk(xin[1]), fqm.at[1], 2)
    partial(0, s0)
    xe = upk(xin[0])
    proj_k(xe, fkv.at[0], 1)
    s1 = partial_scores(1)
    proj_vt(xe, fkv.at[0])
    partial(1, s1)

    own_update((fb,), lambda b: [fkv.at[0], fkv.at[1]], False)
    rwait(kvin, 2)
    own_update((sb,), lambda b: [kvin.at[0], kvin.at[1]], False)

    def prep(b):
        rem = sin_[b]
        own = ml[b]
        mn = jnp.maximum(own, rem)
        a_o = jnp.exp2(own - mn)
        a_r = jnp.exp2(rem - mn)
        inv = 1.0 / (a_o * pltpu.roll(own, 4, 0) + a_r * pltpu.roll(rem, 4, 0))
        f_o, f_r = a_o * inv, a_r * inv
        for p in range(2):
            c_t = jnp.concatenate([acc[b, g * DH:(g + 1) * DH, :] * f_o[g:g + 1, :]
                                   for g in (2 * p, 2 * p + 1)], axis=0)
            r_t = jnp.concatenate([jnp.broadcast_to(f_r[g:g + 1, :], (DH, SL))
                                   for g in (2 * p, 2 * p + 1)], axis=0)
            cown[b, :, p * 128:(p + 1) * 128] = c_t.T
            frem[b, :, p * 128:(p + 1) * 128] = r_t.T

    rwait(sin_, 3 + NPC)
    for b in range(2):
        prep(b)

    def out_rows(c):
        r0, r1 = PQ[c], PQ[c + 1]
        ctx = jnp.concatenate(
            [cown[b, r0:r1, :] + upk(pin[b, r0 // 2:r1 // 2, :]).astype(F32) * frem[b, r0:r1, :] for b in range(2)],
            axis=0).astype(BF16)
        o = jnp.dot(ctx, upk(wob[...]), preferred_element_type=F32)
        for b in range(2):
            o_ref[b, r0:r1, :] = o[b * (r1 - r0):(b + 1) * (r1 - r0)]

    for c in range(NPC):
        if c == NPC - 1:
            for cp in list(sx.values()) + skv + sst + spt[0] + spt[1]:
                cp.wait_send()
        rwait(pin.at[:, prows(c)], 3 + c)
        out_rows(c)


def pallas_dist_rope_attn_qseq_b2_sq128_d512_hq4_dh64_kernel(x, Wq, Wk, Wv, Wo):
    return pl.pallas_call(
        _kernel,
        out_shape=jax.ShapeDtypeStruct((B, SL, D), F32),
        in_specs=[pl.BlockSpec(memory_space=pl.ANY)] * 5,
        out_specs=pl.BlockSpec(memory_space=pltpu.VMEM),
        scratch_shapes=[
            pltpu.VMEM((B, SL, D), F32),
            pltpu.VMEM((D, HD), F32),
            pltpu.VMEM((D, HD), F32),
            pltpu.VMEM((D, HD), F32),
            pltpu.VMEM((HD, D), F32),
            pltpu.VMEM((B, SL // 2, D), U32),
            pltpu.VMEM((D // 2, HD), U32),
            pltpu.VMEM((D // 2, HD), U32),
            pltpu.VMEM((HD // 2, D), U32),
            pltpu.VMEM((HD // 2, D), U32),
            pltpu.VMEM((3, 2, SL, 128), F32),
            pltpu.VMEM((2, 2, SL // 2, HD), U32),
            pltpu.VMEM((2, 2, 2, SL // 2, 128), U32),
            pltpu.VMEM((2, SL // 2, D), U32),
            pltpu.VMEM((2, 2, SL // 2, HD), U32),
            pltpu.VMEM((2, 2, SL // 2, HD), U32),
            pltpu.VMEM((2, 2, 2, SL // 2, 128), U32),
            pltpu.VMEM((2, HD, SL), F32),
            pltpu.VMEM((2, 8, SL), F32),
            pltpu.VMEM((2, SL // 2, HD), U32),
            pltpu.VMEM((2, SL // 2, HD), U32),
            pltpu.VMEM((2, 8, SL), F32),
            pltpu.VMEM((2, 8, SL), F32),
            pltpu.VMEM((2, SL, HD), F32),
            pltpu.VMEM((2, SL, HD), F32),
            pltpu.SemaphoreType.DMA,
            pltpu.SemaphoreType.DMA((4 + NPC,)),
            pltpu.SemaphoreType.REGULAR,
        ],
        compiler_params=pltpu.CompilerParams(collective_id=0),
    )(x, Wq, Wk, Wv, Wo)
```
